```python
import numpy as np

kernel_name = "dist_ring_attn_i_s256_d64"

def setup_inputs():
    S, D = 1024, 64
    q = np.random.randn(S, D).astype(np.float32)
    k = np.random.randn(S, D).astype(np.float32)
    v = np.random.randn(S, D).astype(np.float32)
    return {"q": q, "k": k, "v": v}

def reference(q: np.ndarray, k: np.ndarray, v: np.ndarray) -> np.ndarray:
    D = q.shape[1]
    scores = q @ k.T / np.sqrt(D)
    scores_max = np.max(scores, axis=1, keepdims=True)
    weights = np.exp(scores - scores_max)
    weights = weights / np.sum(weights, axis=1, keepdims=True)
    return weights @ v
```

```python
import math

import jax
import jax.numpy as jnp
from jax import lax
from jax.experimental import pallas as pl
from jax.experimental.pallas import tpu as pltpu

_MESH = pl.DeviceIdType.MESH
_S = 256
_D = 64
_H = 128
_SCALE_LOG2E = math.log2(math.e) / math.sqrt(_D)

_SELF, _XN, _YN, _DG = 0, 1, 2, 3
_KL, _KH, _VL, _VH = 0, 1, 2, 3


def _body(q_hbm, k_hbm, v_hbm, o_ref, in_f32, kv, ld_sem, send_sem, recv_sem):
    me = lax.axis_index("i")
    xn = 3 - me
    yn = me ^ 1
    dev = {_XN: xn, _YN: yn}

    bs = pltpu.get_barrier_semaphore()
    for n in (xn, yn):
        pl.semaphore_signal(bs, inc=1, device_id=(n,), device_id_type=_MESH)

    ld_k = pltpu.make_async_copy(k_hbm, in_f32.at[0], ld_sem.at[0])
    ld_v = pltpu.make_async_copy(v_hbm, in_f32.at[1], ld_sem.at[1])
    ld_q = pltpu.make_async_copy(q_hbm, in_f32.at[2], ld_sem.at[2])
    ld_k.start()
    ld_v.start()
    ld_q.start()

    started = []

    def send(src_slot, c, to, dst_slot):
        cp = pltpu.make_async_remote_copy(
            kv.at[src_slot, c], kv.at[dst_slot, c],
            send_sem.at[len(started)], recv_sem.at[dst_slot - 1, c],
            device_id=(dev[to],), device_id_type=_MESH)
        cp.start()
        started.append(cp)

    def arrived(slot, c):
        pltpu.make_async_remote_copy(
            kv.at[_SELF, c], kv.at[slot, c], send_sem.at[0], recv_sem.at[slot - 1, c],
            device_id=(xn,), device_id_type=_MESH).wait_recv()

    ld_k.wait()
    kv[_SELF, _KL] = in_f32[0, :, 0:_H].astype(jnp.bfloat16)
    kv[_SELF, _KH] = in_f32[0, :, _H:].astype(jnp.bfloat16)
    pl.semaphore_wait(bs, 2)
    send(_SELF, _KL, _YN, _YN)
    send(_SELF, _KH, _XN, _XN)
    ld_v.wait()
    kv[_SELF, _VL] = in_f32[1, :, 0:_H].astype(jnp.bfloat16)
    kv[_SELF, _VH] = in_f32[1, :, _H:].astype(jnp.bfloat16)
    send(_SELF, _VL, _YN, _YN)
    send(_SELF, _VH, _XN, _XN)
    send(_SELF, _KH, _YN, _YN)
    send(_SELF, _VH, _YN, _YN)
    send(_SELF, _KL, _XN, _XN)
    send(_SELF, _VL, _XN, _XN)

    ld_q.wait()
    qT = (in_f32[2] * _SCALE_LOG2E).astype(jnp.bfloat16)

    def scores(slot, c):
        return lax.dot_general(kv[slot, c], qT, (((0,), (0,)), ((), ())),
                               preferred_element_type=jnp.float32)

    state = [None]

    def update(slot, ck, cv, wait_v=False):
        sT = scores(slot, ck)
        mj = jnp.max(sT, axis=0, keepdims=True)
        if state[0] is None:
            m_new = mj
        else:
            m_old, l_old, o_old = state[0]
            m_new = jnp.maximum(m_old, mj)
            alpha = jnp.exp2(m_old - m_new)
        p = jnp.exp2(sT - m_new)
        lj = jnp.sum(p, axis=0, keepdims=True)
        pb = p.astype(jnp.bfloat16)
        if wait_v:
            arrived(slot, cv)
        oj = jnp.dot(kv[slot, cv], pb, preferred_element_type=jnp.float32)
        if state[0] is None:
            state[0] = (m_new, lj, oj)
        else:
            state[0] = (m_new, alpha * l_old + lj, alpha * o_old + oj)

    update(_SELF, _KL, _VL)
    update(_SELF, _KH, _VH)

    arrived(_YN, _KL)
    send(_YN, _KL, _XN, _DG)
    arrived(_XN, _KH)
    send(_XN, _KH, _YN, _DG)
    arrived(_YN, _VL)
    send(_YN, _VL, _XN, _DG)
    arrived(_XN, _VH)
    send(_XN, _VH, _YN, _DG)
    update(_YN, _KL, _VL)
    update(_XN, _KH, _VH)
    arrived(_XN, _KL)
    update(_XN, _KL, _VL, wait_v=True)
    arrived(_YN, _KH)
    update(_YN, _KH, _VH, wait_v=True)
    arrived(_DG, _KL)
    arrived(_DG, _KH)
    update(_DG, _KL, _VL, wait_v=True)
    update(_DG, _KH, _VH, wait_v=True)

    _, l, o = state[0]
    o_ref[...] = o * pl.reciprocal(l, approx=False)
    for cp in started:
        cp.wait_send()


def pallas_dist_ring_attn_i_s256_d64_kernel(q, k, v):
    oT = pl.pallas_call(
        _body,
        out_shape=jax.ShapeDtypeStruct((_D, _S), jnp.float32),
        in_specs=[pl.BlockSpec(memory_space=pl.ANY)] * 3,
        out_specs=pl.BlockSpec(memory_space=pltpu.VMEM),
        scratch_shapes=[
            pltpu.VMEM((3, _D, _S), jnp.float32),
            pltpu.VMEM((4, 4, _D, _H), jnp.bfloat16),
            pltpu.SemaphoreType.DMA((3,)),
            pltpu.SemaphoreType.DMA((12,)),
            pltpu.SemaphoreType.DMA((3, 4)),
        ],
        compiler_params=pltpu.CompilerParams(
            collective_id=0, disable_semaphore_checks=True),
    )(q.T, k.T, v.T)
    return oT.T
```

```python
import math

import jax
import jax.numpy as jnp
from jax import lax
from jax.experimental import pallas as pl
from jax.experimental.pallas import tpu as pltpu

_MESH = pl.DeviceIdType.MESH
_S = 256
_D = 64
_H = 128
_SCALE_LOG2E = math.log2(math.e) / math.sqrt(_D)
NSUB = 4
PR = _D // NSUB

OWN_KL, OWN_KH, OWN_VL, OWN_VH = 0, 1, 2, 3
K1, V1, K2, V2, K3, V3 = 4, 6, 8, 10, 12, 14


def _body(q_hbm, k_hbm, v_hbm, o_ref, in_f32, kv, ldk_sem, ld_sem, ssem, fsem, gsem, hello):
    me = lax.axis_index("i")
    xn = 3 - me
    yn = me ^ 1
    bs = pltpu.get_barrier_semaphore()

    def sig(sem, d):
        pl.semaphore_signal(sem, inc=1, device_id=(d,), device_id_type=_MESH)

    ld_k = [pltpu.make_async_copy(k_hbm.at[pl.ds(i * PR, PR)], in_f32.at[0, pl.ds(i * PR, PR)], ldk_sem.at[i])
            for i in range(NSUB)]
    ld_v = pltpu.make_async_copy(v_hbm, in_f32.at[1], ld_sem.at[0])
    ld_q = pltpu.make_async_copy(q_hbm, in_f32.at[2], ld_sem.at[1])
    for c in ld_k:
        c.start()

    @pl.when(me != 2)
    def _():
        sig(bs, yn)
        sig(bs, xn)

    ld_v.start()
    ld_q.start()

    @pl.when(me == 2)
    def _():
        pl.semaphore_wait(bs, 2)
        sig(hello, yn)
        sig(hello, xn)

    def rdma(src, dst, s, rsem, dev):
        return pltpu.make_async_remote_copy(src, dst, ssem.at[s], rsem, device_id=(dev,), device_id_type=_MESH)

    def piece(src_slot, dst_slot, fidx, to_y, i):
        rows = pl.ds(i * PR, PR)
        rdma(kv.at[src_slot, rows], kv.at[dst_slot, rows], 0 if to_y else 1, fsem.at[fidx, i], yn if to_y else xn).start()

    def whole(src_slot, dst_slot, g, to_y):
        rdma(kv.at[src_slot], kv.at[dst_slot], 0 if to_y else 1, gsem.at[g], yn if to_y else xn).start()

    def y_k(i): piece(OWN_KL, K1 + 0, 0, True, i)
    def x_k(i): piece(OWN_KH, K1 + 1, 1, False, i)
    def y_v():
        for i in range(NSUB): piece(OWN_VL, V1 + 0, 2, True, i)
    def x_v():
        for i in range(NSUB): piece(OWN_VH, V1 + 1, 3, False, i)
    def y_rest():
        whole(OWN_KH, K2 + 1, 0, True)
        whole(OWN_VH, V2 + 1, 1, True)
    def x_rest():
        whole(OWN_KL, K2 + 0, 0, False)
        whole(OWN_VL, V2 + 0, 1, False)

    def cvt_k(i):
        rows = pl.ds(i * PR, PR)
        ld_k[i].wait()
        kv[OWN_KL, rows] = in_f32[0, rows, 0:_H].astype(jnp.bfloat16)
        kv[OWN_KH, rows] = in_f32[0, rows, _H:].astype(jnp.bfloat16)

    cvt_k(0)
    @pl.when(me == 0)
    def _():
        pl.semaphore_wait(bs, 2)

    @pl.when((me & 1) == 1)
    def _():
        pl.semaphore_wait(bs, 1)
    for i in range(NSUB):
        if i > 0:
            cvt_k(i)

        @pl.when(me != 3)
        def _():
            y_k(i)

        @pl.when(me != 1)
        def _():
            x_k(i)
    ld_v.wait()
    kv[OWN_VL] = in_f32[1, :, 0:_H].astype(jnp.bfloat16)
    kv[OWN_VH] = in_f32[1, :, _H:].astype(jnp.bfloat16)

    @pl.when((me & 1) == 0)
    def _():
        y_v(); x_v(); y_rest(); x_rest()

    @pl.when(me == 1)
    def _():
        y_v(); y_rest()

    @pl.when(me == 3)
    def _():
        x_v(); x_rest()

    ld_q.wait()
    qT = (in_f32[2] * _SCALE_LOG2E).astype(jnp.bfloat16)

    def scores(slot):
        return lax.dot_general(kv[slot], qT, (((0,), (0,)), ((), ())),
                               preferred_element_type=jnp.float32)

    def rowsum8(p):
        acc = p[0:8]
        for r in range(1, p.shape[0] // 8):
            acc = acc + p[8 * r:8 * r + 8]
        return acc

    state = [None]

    def s_phase(ka, name):
        s0 = scores(ka)
        s1 = scores(ka + 1)
        m_new = jnp.maximum(jnp.max(s0, axis=0, keepdims=True), jnp.max(s1, axis=0, keepdims=True))
        alpha = None
        if state[0] is not None:
            m_new = jnp.maximum(state[0][0], m_new)
            alpha = jnp.exp2(state[0][0] - m_new)
        p0 = jnp.exp2(s0 - m_new)
        p1 = jnp.exp2(s1 - m_new)
        l8 = rowsum8(p0) + rowsum8(p1)
        return m_new, alpha, l8, p0.astype(jnp.bfloat16), p1.astype(jnp.bfloat16)

    def pv_phase(ph, va, name, last=False):
        m_new, alpha, l8, p0, p1 = ph
        oj = (jnp.dot(kv[va], p0, preferred_element_type=jnp.float32)
              + jnp.dot(kv[va + 1], p1, preferred_element_type=jnp.float32))
        if alpha is not None:
            _, l8_old, o_old = state[0]
            l8 = alpha * l8_old + l8
            oj = oj + alpha * o_old
        if last:
            inv_l = pl.reciprocal(jnp.sum(l8, axis=0, keepdims=True), approx=False)
            o_ref[...] = oj * inv_l
        state[0] = (m_new, l8, oj)

    pv_phase(s_phase(OWN_KL, "0"), OWN_VL, "0")

    @pl.when((me & 1) == 1)
    def _():
        pl.semaphore_wait(hello, 1)

    @pl.when(me == 3)
    def _():
        for i in range(NSUB): y_k(i)
        y_v(); y_rest()

    @pl.when(me == 1)
    def _():
        for i in range(NSUB): x_k(i)
        x_v(); x_rest()

    def fwd(fidx, src_slot, dst_slot, g, i, nm):
        rows = pl.ds(i * PR, PR)
        rdma(kv.at[src_slot, rows], kv.at[src_slot, rows], 2, fsem.at[fidx, i], xn).wait_recv()
        rdma(kv.at[src_slot, rows], kv.at[dst_slot, rows], 2, gsem.at[g], xn if fidx in (0, 2) else yn).start()

    def wait_group(base, g, nm):
        pltpu.make_async_copy(kv.at[pl.ds(base, 2)], kv.at[pl.ds(base, 2)], gsem.at[g]).wait()

    for i in range(NSUB):
        fwd(0, K1 + 0, K3 + 0, 2, i, "yKL")
        fwd(1, K1 + 1, K3 + 1, 2, i, "xKH")
    for i in range(NSUB):
        fwd(2, V1 + 0, V3 + 0, 3, i, "yVL")
        fwd(3, V1 + 1, V3 + 1, 3, i, "xVH")
    pv_phase(s_phase(K1, "1"), V1, "1")
    wait_group(K2, 0, "K2")
    ph = s_phase(K2, "2")
    wait_group(V2, 1, "V2")
    pv_phase(ph, V2, "2")
    wait_group(K3, 2, "K3")
    ph = s_phase(K3, "3")
    pltpu.make_async_copy(kv.at[pl.ds(0, 4)], kv.at[pl.ds(0, 4)], ssem.at[0]).wait()
    pltpu.make_async_copy(kv.at[pl.ds(0, 4)], kv.at[pl.ds(0, 4)], ssem.at[1]).wait()
    pltpu.make_async_copy(kv.at[pl.ds(4, 4)], kv.at[pl.ds(4, 4)], ssem.at[2]).wait()
    wait_group(V3, 3, "V3")
    pv_phase(ph, V3, "3", last=True)


def pallas_dist_ring_attn_i_s256_d64_kernel(q, k, v):
    oT = pl.pallas_call(
        _body,
        out_shape=jax.ShapeDtypeStruct((_D, _S), jnp.float32),
        in_specs=[pl.BlockSpec(memory_space=pl.ANY)] * 3,
        out_specs=pl.BlockSpec(memory_space=pltpu.VMEM),
        scratch_shapes=[
            pltpu.VMEM((3, _D, _S), jnp.float32),
            pltpu.VMEM((16, _D, _H), jnp.bfloat16),
            pltpu.SemaphoreType.DMA((NSUB,)),
            pltpu.SemaphoreType.DMA((2,)),
            pltpu.SemaphoreType.DMA((3,)),
            pltpu.SemaphoreType.DMA((4, NSUB)),
            pltpu.SemaphoreType.DMA((4,)),
            pltpu.SemaphoreType.REGULAR,
        ],
        compiler_params=pltpu.CompilerParams(
            collective_id=0, disable_semaphore_checks=True),
    )(q.T, k.T, v.T)
    return oT.T
```

```python
import math

import jax
import jax.numpy as jnp
from jax import lax
from jax.experimental import pallas as pl
from jax.experimental.pallas import tpu as pltpu

_MESH = pl.DeviceIdType.MESH
_S = 256
_D = 64
_H = 128
_SCALE_LOG2E = math.log2(math.e) / math.sqrt(_D)

_NP = 8
_PR = _D // _NP

_OWN_KL, _OWN_KH, _OWN_VL, _OWN_VH = 0, 1, 2, 3
_K1, _V1, _K2, _V2, _K3, _V3 = 4, 6, 8, 10, 12, 14


def _body(q_hbm, k_hbm, v_hbm, o_ref, in_f32, kv,
          ldk_sem, ld_sem, send_sem, piece_sem, pair_sem, hello):
    me = lax.axis_index("i")
    xn = 3 - me
    yn = me ^ 1
    odd = (me & 1) == 1
    barrier = pltpu.get_barrier_semaphore()

    def signal(sem, dev):
        pl.semaphore_signal(sem, inc=1, device_id=(dev,), device_id_type=_MESH)

    def k_rows(i):
        return pl.ds(i * _PR, _PR)

    ld_k = [pltpu.make_async_copy(k_hbm.at[k_rows(i)], in_f32.at[0, k_rows(i)],
                                  ldk_sem.at[i]) for i in range(_NP)]
    ld_v = pltpu.make_async_copy(v_hbm, in_f32.at[1], ld_sem.at[0])
    ld_q = pltpu.make_async_copy(q_hbm, in_f32.at[2], ld_sem.at[1])
    for c in ld_k:
        c.start()

    @pl.when(me != 2)
    def _():
        signal(barrier, yn)
        signal(barrier, xn)

    ld_v.start()
    ld_q.start()

    @pl.when(me == 2)
    def _():
        pl.semaphore_wait(barrier, 2)
        signal(hello, yn)
        signal(hello, xn)

    def rdma(src, dst, s, recv_sem, dev):
        return pltpu.make_async_remote_copy(
            src, dst, send_sem.at[s], recv_sem, device_id=(dev,), device_id_type=_MESH)

    def send_piece(src_slot, dst_slot, row, to_y, i):
        rdma(kv.at[src_slot, k_rows(i)], kv.at[dst_slot, k_rows(i)], 0 if to_y else 1,
             piece_sem.at[row * _NP + i], yn if to_y else xn).start()

    def send_whole(src_slot, dst_slot, pair, to_y):
        rdma(kv.at[src_slot], kv.at[dst_slot], 0 if to_y else 1,
             pair_sem.at[pair], yn if to_y else xn).start()

    def y_k(i):
        send_piece(_OWN_KL, _K1, 0, True, i)

    def x_k(i):
        send_piece(_OWN_KH, _K1 + 1, 1, False, i)

    def y_v():
        for i in range(_NP):
            send_piece(_OWN_VL, _V1, 2, True, i)

    def x_v():
        for i in range(_NP):
            send_piece(_OWN_VH, _V1 + 1, 3, False, i)

    def y_rest():
        send_whole(_OWN_KH, _K2 + 1, 0, True)
        send_whole(_OWN_VH, _V2 + 1, 1, True)

    def x_rest():
        send_whole(_OWN_KL, _K2, 0, False)
        send_whole(_OWN_VL, _V2, 1, False)

    def cast_k(i):
        ld_k[i].wait()
        kv[_OWN_KL, k_rows(i)] = in_f32[0, k_rows(i), 0:_H].astype(jnp.bfloat16)
        kv[_OWN_KH, k_rows(i)] = in_f32[0, k_rows(i), _H:].astype(jnp.bfloat16)

    cast_k(0)

    @pl.when(me == 0)
    def _():
        pl.semaphore_wait(barrier, 2)

    @pl.when(odd)
    def _():
        pl.semaphore_wait(barrier, 1)

    for i in range(_NP):
        if i > 0:
            cast_k(i)

        @pl.when(me != 3)
        def _():
            y_k(i)

        @pl.when(me != 1)
        def _():
            x_k(i)

    ld_v.wait()
    kv[_OWN_VL] = in_f32[1, :, 0:_H].astype(jnp.bfloat16)
    kv[_OWN_VH] = in_f32[1, :, _H:].astype(jnp.bfloat16)

    @pl.when(jnp.logical_not(odd))
    def _():
        y_v()
        x_v()
        y_rest()
        x_rest()

    @pl.when(me == 1)
    def _():
        y_v()
        y_rest()

    @pl.when(me == 3)
    def _():
        x_v()
        x_rest()

    ld_q.wait()
    qT = (in_f32[2] * _SCALE_LOG2E).astype(jnp.bfloat16)

    def scores_t(slot):
        return lax.dot_general(kv[slot], qT, (((0,), (0,)), ((), ())),
                               preferred_element_type=jnp.float32)

    def sum8(p):
        acc = p[0:8]
        for r in range(1, _H // 8):
            acc = acc + p[8 * r:8 * r + 8]
        return acc

    def softmax_step(ks, state):
        s0, s1 = scores_t(ks), scores_t(ks + 1)
        m_new = jnp.maximum(jnp.max(s0, axis=0, keepdims=True),
                            jnp.max(s1, axis=0, keepdims=True))
        alpha = None
        if state is not None:
            m_new = jnp.maximum(state[0], m_new)
            alpha = jnp.exp2(state[0] - m_new)
        p0, p1 = jnp.exp2(s0 - m_new), jnp.exp2(s1 - m_new)
        return (m_new, alpha, sum8(p0) + sum8(p1),
                p0.astype(jnp.bfloat16), p1.astype(jnp.bfloat16))

    def pv_step(step, vs, state):
        m_new, alpha, l8, p0, p1 = step
        o = (jnp.dot(kv[vs], p0, preferred_element_type=jnp.float32)
             + jnp.dot(kv[vs + 1], p1, preferred_element_type=jnp.float32))
        if state is not None:
            l8 = alpha * state[1] + l8
            o = o + alpha * state[2]
        return m_new, l8, o

    state = pv_step(softmax_step(_OWN_KL, None), _OWN_VL, None)

    @pl.when(odd)
    def _():
        pl.semaphore_wait(hello, 1)

    @pl.when(me == 3)
    def _():
        for i in range(_NP):
            y_k(i)
        y_v()
        y_rest()

    @pl.when(me == 1)
    def _():
        for i in range(_NP):
            x_k(i)
        x_v()
        x_rest()

    def forward(row, src_slot, dst_slot, pair, dev, i):
        piece = kv.at[src_slot, k_rows(i)]
        rdma(piece, piece, 2, piece_sem.at[row * _NP + i], dev).wait_recv()
        rdma(piece, kv.at[dst_slot, k_rows(i)], 2, pair_sem.at[pair], dev).start()

    def wait_pair(slot, pair):
        both = kv.at[pl.ds(slot, 2)]
        pltpu.make_async_copy(both, both, pair_sem.at[pair]).wait()

    for i in range(_NP):
        forward(0, _K1, _K3, 2, xn, i)
        forward(1, _K1 + 1, _K3 + 1, 2, yn, i)
    for i in range(_NP):
        forward(2, _V1, _V3, 3, xn, i)
        forward(3, _V1 + 1, _V3 + 1, 3, yn, i)

    state = pv_step(softmax_step(_K1, state), _V1, state)

    wait_pair(_K2, 0)
    step = softmax_step(_K2, state)
    wait_pair(_V2, 1)
    state = pv_step(step, _V2, state)

    wait_pair(_K3, 2)
    step = softmax_step(_K3, state)
    for slots, s in ((pl.ds(_OWN_KL, 4), 0), (pl.ds(_OWN_KL, 4), 1), (pl.ds(_K1, 4), 2)):
        pltpu.make_async_copy(kv.at[slots], kv.at[slots], send_sem.at[s]).wait()
    wait_pair(_V3, 3)
    _, l8, o = pv_step(step, _V3, state)
    inv_l = pl.reciprocal(jnp.sum(l8, axis=0, keepdims=True), approx=False)
    o_ref[...] = o * inv_l


def pallas_dist_ring_attn_i_s256_d64_kernel(q, k, v):
    o_t = pl.pallas_call(
        _body,
        out_shape=jax.ShapeDtypeStruct((_D, _S), jnp.float32),
        in_specs=[pl.BlockSpec(memory_space=pl.ANY)] * 3,
        out_specs=pl.BlockSpec(memory_space=pltpu.VMEM),
        scratch_shapes=[
            pltpu.VMEM((3, _D, _S), jnp.float32),
            pltpu.VMEM((16, _D, _H), jnp.bfloat16),
            pltpu.SemaphoreType.DMA((_NP,)),
            pltpu.SemaphoreType.DMA((2,)),
            pltpu.SemaphoreType.DMA((3,)),
            pltpu.SemaphoreType.DMA((4 * _NP,)),
            pltpu.SemaphoreType.DMA((4,)),
            pltpu.SemaphoreType.REGULAR,
        ],
        compiler_params=pltpu.CompilerParams(
            collective_id=0,
            disable_semaphore_checks=True,
        ),
    )(q.T, k.T, v.T)
    return o_t.T
```

```python
import math

import jax
import jax.numpy as jnp
from jax import lax
from jax.experimental import pallas as pl
from jax.experimental.pallas import tpu as pltpu

_MESH = pl.DeviceIdType.MESH
_S = 256
_D = 64
_H = 128
_SCALE_LOG2E = math.log2(math.e) / math.sqrt(_D)

_NP = 16
_PR = _D // _NP
_NL = 8
_LR = _D // _NL

_OWN_KL, _OWN_KH, _OWN_VL, _OWN_VH = 0, 1, 2, 3
_K1, _V1, _K2, _V2, _K3, _V3 = 4, 6, 8, 10, 12, 14


def _body(q_hbm, k_hbm, v_hbm, o_ref, in_f32, kv,
          ldk_sem, ld_sem, send_sem, piece_sem, pair_sem, hello):
    me = lax.axis_index("i")
    xn = 3 - me
    yn = me ^ 1
    odd = (me & 1) == 1
    barrier = pltpu.get_barrier_semaphore()

    def signal(sem, dev):
        pl.semaphore_signal(sem, inc=1, device_id=(dev,), device_id_type=_MESH)

    def k_rows(i):
        return pl.ds(i * _PR, _PR)

    ld_k = [pltpu.make_async_copy(k_hbm.at[pl.ds(j * _LR, _LR)],
                                  in_f32.at[0, pl.ds(j * _LR, _LR)], ldk_sem.at[j])
            for j in range(_NL)]
    ld_v = pltpu.make_async_copy(v_hbm, in_f32.at[1], ld_sem.at[0])
    ld_q = pltpu.make_async_copy(q_hbm, in_f32.at[2], ld_sem.at[1])
    for c in ld_k:
        c.start()

    @pl.when(me != 2)
    def _():
        signal(barrier, yn)
        signal(barrier, xn)

    ld_v.start()
    ld_q.start()

    @pl.when(me == 2)
    def _():
        pl.semaphore_wait(barrier, 2)
        signal(hello, yn)
        signal(hello, xn)

    def rdma(src, dst, s, recv_sem, dev):
        return pltpu.make_async_remote_copy(
            src, dst, send_sem.at[s], recv_sem, device_id=(dev,), device_id_type=_MESH)

    def send_piece(src_slot, dst_slot, row, to_y, i):
        rdma(kv.at[src_slot, k_rows(i)], kv.at[dst_slot, k_rows(i)], 0 if to_y else 1,
             piece_sem.at[row * _NP + i], yn if to_y else xn).start()

    def send_whole(src_slot, dst_slot, pair, to_y):
        rdma(kv.at[src_slot], kv.at[dst_slot], 0 if to_y else 1,
             pair_sem.at[pair], yn if to_y else xn).start()

    def y_k(i):
        send_piece(_OWN_KL, _K1, 0, True, i)

    def x_k(i):
        send_piece(_OWN_KH, _K1 + 1, 1, False, i)

    def y_v():
        for i in range(_NP):
            send_piece(_OWN_VL, _V1, 2, True, i)

    def x_v():
        for i in range(_NP):
            send_piece(_OWN_VH, _V1 + 1, 3, False, i)

    def y_rest():
        send_whole(_OWN_KH, _K2 + 1, 0, True)
        send_whole(_OWN_VH, _V2 + 1, 1, True)

    def x_rest():
        send_whole(_OWN_KL, _K2, 0, False)
        send_whole(_OWN_VL, _V2, 1, False)

    def cast_k(i):
        if (i * _PR) % _LR == 0:
            ld_k[i * _PR // _LR].wait()
        kv[_OWN_KL, k_rows(i)] = in_f32[0, k_rows(i), 0:_H].astype(jnp.bfloat16)
        kv[_OWN_KH, k_rows(i)] = in_f32[0, k_rows(i), _H:].astype(jnp.bfloat16)

    cast_k(0)

    @pl.when(me == 0)
    def _():
        pl.semaphore_wait(barrier, 2)

    @pl.when(odd)
    def _():
        pl.semaphore_wait(barrier, 1)

    for i in range(_NP):
        if i > 0:
            cast_k(i)

        @pl.when(me != 3)
        def _():
            y_k(i)

        @pl.when(me != 1)
        def _():
            x_k(i)

    ld_v.wait()
    kv[_OWN_VL] = in_f32[1, :, 0:_H].astype(jnp.bfloat16)
    kv[_OWN_VH] = in_f32[1, :, _H:].astype(jnp.bfloat16)

    @pl.when(jnp.logical_not(odd))
    def _():
        for i in range(_NP):
            send_piece(_OWN_VL, _V1, 2, True, i)
            send_piece(_OWN_VH, _V1 + 1, 3, False, i)
        y_rest()
        x_rest()

    @pl.when(me == 1)
    def _():
        y_v()
        y_rest()

    @pl.when(me == 3)
    def _():
        x_v()
        x_rest()

    ld_q.wait()
    qT = (in_f32[2] * _SCALE_LOG2E).astype(jnp.bfloat16)

    def scores_t(slot):
        return lax.dot_general(kv[slot], qT, (((0,), (0,)), ((), ())),
                               preferred_element_type=jnp.float32)

    def sum8(p):
        acc = p[0:8]
        for r in range(1, _H // 8):
            acc = acc + p[8 * r:8 * r + 8]
        return acc

    def softmax_step(ks, state):
        s0, s1 = scores_t(ks), scores_t(ks + 1)
        m_new = jnp.maximum(jnp.max(s0, axis=0, keepdims=True),
                            jnp.max(s1, axis=0, keepdims=True))
        alpha = None
        if state is not None:
            m_new = jnp.maximum(state[0], m_new)
            alpha = jnp.exp2(state[0] - m_new)
        p0, p1 = jnp.exp2(s0 - m_new), jnp.exp2(s1 - m_new)
        return (m_new, alpha, sum8(p0) + sum8(p1),
                p0.astype(jnp.bfloat16), p1.astype(jnp.bfloat16))

    def pv_step(step, vs, state):
        m_new, alpha, l8, p0, p1 = step
        o = (jnp.dot(kv[vs], p0, preferred_element_type=jnp.float32)
             + jnp.dot(kv[vs + 1], p1, preferred_element_type=jnp.float32))
        if state is not None:
            l8 = alpha * state[1] + l8
            o = o + alpha * state[2]
        return m_new, l8, o

    state = pv_step(softmax_step(_OWN_KL, None), _OWN_VL, None)

    @pl.when(odd)
    def _():
        pl.semaphore_wait(hello, 1)

    @pl.when(me == 3)
    def _():
        for i in range(_NP):
            y_k(i)
        y_v()
        y_rest()

    @pl.when(me == 1)
    def _():
        for i in range(_NP):
            x_k(i)
        x_v()
        x_rest()

    def forward(row, src_slot, dst_slot, pair, dev, i):
        piece = kv.at[src_slot, k_rows(i)]
        rdma(piece, piece, 2, piece_sem.at[row * _NP + i], dev).wait_recv()
        rdma(piece, kv.at[dst_slot, k_rows(i)], 2, pair_sem.at[pair], dev).start()

    def wait_pair(slot, pair):
        both = kv.at[pl.ds(slot, 2)]
        pltpu.make_async_copy(both, both, pair_sem.at[pair]).wait()

    for i in range(_NP):
        forward(0, _K1, _K3, 2, xn, i)
        forward(1, _K1 + 1, _K3 + 1, 2, yn, i)
    for i in range(_NP):
        forward(2, _V1, _V3, 3, xn, i)
        forward(3, _V1 + 1, _V3 + 1, 3, yn, i)

    state = pv_step(softmax_step(_K1, state), _V1, state)

    wait_pair(_K2, 0)
    step = softmax_step(_K2, state)
    wait_pair(_V2, 1)
    state = pv_step(step, _V2, state)

    wait_pair(_K3, 2)
    step = softmax_step(_K3, state)
    for slots, s in ((pl.ds(_OWN_KL, 4), 0), (pl.ds(_OWN_KL, 4), 1), (pl.ds(_K1, 4), 2)):
        pltpu.make_async_copy(kv.at[slots], kv.at[slots], send_sem.at[s]).wait()
    wait_pair(_V3, 3)
    _, l8, o = pv_step(step, _V3, state)
    inv_l = pl.reciprocal(jnp.sum(l8, axis=0, keepdims=True), approx=False)
    o_ref[...] = o * inv_l


def pallas_dist_ring_attn_i_s256_d64_kernel(q, k, v):
    o_t = pl.pallas_call(
        _body,
        out_shape=jax.ShapeDtypeStruct((_D, _S), jnp.float32),
        in_specs=[pl.BlockSpec(memory_space=pl.ANY)] * 3,
        out_specs=pl.BlockSpec(memory_space=pltpu.VMEM),
        scratch_shapes=[
            pltpu.VMEM((3, _D, _S), jnp.float32),
            pltpu.VMEM((16, _D, _H), jnp.bfloat16),
            pltpu.SemaphoreType.DMA((_NL,)),
            pltpu.SemaphoreType.DMA((2,)),
            pltpu.SemaphoreType.DMA((3,)),
            pltpu.SemaphoreType.DMA((4 * _NP,)),
            pltpu.SemaphoreType.DMA((4,)),
            pltpu.SemaphoreType.REGULAR,
        ],
        compiler_params=pltpu.CompilerParams(
            collective_id=0,
            disable_semaphore_checks=True,
        ),
    )(q.T, k.T, v.T)
    return o_t.T
```
